```python
import numpy as np

kernel_name = "dist_ag_xy_y_m1024_n512"

def setup_inputs():
    return {"x": np.random.randn(2048, 512).astype(np.float32)}

def reference(x: np.ndarray) -> np.ndarray:
    return x
```

```python
import jax
import jax.numpy as jnp
from jax import lax
from jax.experimental import pallas as pl
from jax.experimental.pallas import tpu as pltpu

_MESH = pl.DeviceIdType.MESH

_TILE = 16
_FWD_CHUNKS = (16,) * 29
_BOTH_CHUNKS = (64, 16, 16)
_LOAD_GROUPS = (1, 1, 2, 6)
_SEND_AHEAD = 160
_X_LAG = 96


def _schedule():
    chunks, start = [], 0
    for size in _FWD_CHUNKS + _BOTH_CHUNKS:
        chunks.append((start, size))
        start += size
    events = []
    for i, (s, c) in enumerate(chunks):
        events.append((s + c, 0, "recv_y", i))
        events.append((s - _SEND_AHEAD, 1, "send_y", i))
        if i < len(_FWD_CHUNKS):
            events.append((s + c + _X_LAG, 2, "recv_x", i))
    return chunks, [(kind, i) for _, _, kind, i in sorted(events)]


def pallas_dist_ag_xy_y_m1024_n512_kernel(x: jax.Array):
    m, n = x.shape
    chunks, events = _schedule()
    n_fwd = len(_FWD_CHUNKS)
    fwd_rows = sum(_FWD_CHUNKS)
    y_rows = fwd_rows + sum(_BOTH_CHUNKS)
    assert fwd_rows + y_rows == m

    groups, first = {}, 0
    for count in _LOAD_GROUPS + (len(chunks) - sum(_LOAD_GROUPS),):
        groups[first] = (
            chunks[first][0],
            sum(c for _, c in chunks[first : first + count]),
        )
        first += count

    def body(x_ref, o_ref, buf, load_sems, send_sems, y_sems, x_sems, x_ready):
        my_x, my_y = lax.axis_index("x"), lax.axis_index("y")
        own, other = my_y * m, (1 - my_y) * m
        barrier = pltpu.get_barrier_semaphore()

        def column(cx):
            y_nbr, x_nbr = (cx, 1 - my_y), (1 - cx, my_y)

            def row(col, s, c):
                return s if col == 0 else m - s - c

            def at(base, r, c):
                return pl.ds(pl.multiple_of(base + r, _TILE), c)

            def load(r, c, k):
                return pltpu.make_async_copy(
                    x_ref.at[pl.ds(r, c)], o_ref.at[at(own, r, c)], load_sems.at[k]
                )

            def remote(rows, send_sem, recv_sem, nbr):
                return pltpu.make_async_remote_copy(
                    buf.at[rows], buf.at[rows], send_sem, recv_sem,
                    device_id=nbr, device_id_type=_MESH,
                )

            loads = {
                i: load(row(cx, s, c), c, k) for k, (i, (s, c)) in enumerate(groups.items())
            }
            *early_loads, late_load = loads.values()
            unsent_load = load(row(1 - cx, 0, fwd_rows), fwd_rows, len(groups))
            for copy in early_loads:
                copy.start()

            pl.semaphore_signal(barrier, 1, device_id=y_nbr, device_id_type=_MESH)
            if cx == 0:
                pl.semaphore_signal(barrier, 1, device_id=x_nbr, device_id_type=_MESH)

            for kind, i in events:
                s, c = chunks[i]
                if kind == "send_y":
                    rows = at(own, row(cx, s, c), c)
                    if i in loads:
                        loads[i].wait()
                    if i == 0:
                        late_load.start()
                        unsent_load.start()
                    buf[rows, :] = o_ref[rows, :].astype(jnp.bfloat16)
                    if i == 0:
                        pl.semaphore_wait(barrier, 1 + cx)
                    remote(rows, send_sems.at[0], y_sems.at[i], y_nbr).start()
                    if i == 0 and cx == 1:
                        pl.semaphore_signal(
                            x_ready, 1, device_id=x_nbr, device_id_type=_MESH
                        )
                    continue
                if kind == "recv_y":
                    rows = at(other, row(cx, s, c), c)
                    if i == 0 and cx == 0:
                        pl.semaphore_wait(x_ready, 1)
                    remote(rows, send_sems.at[0], y_sems.at[i], y_nbr).wait_recv()
                    if i < n_fwd:
                        remote(rows, send_sems.at[1], x_sems.at[i], x_nbr).start()
                else:
                    rows = at(other, row(1 - cx, s, c), c)
                    remote(rows, send_sems.at[1], x_sems.at[i], x_nbr).wait_recv()
                o_ref[rows, :] = buf[rows, :].astype(o_ref.dtype)

            unsent_load.wait()
            for k, (base, c) in enumerate(((own, y_rows), (other, fwd_rows))):
                sent = buf.at[at(base, row(cx, 0, c), c)]
                pltpu.make_async_copy(sent, sent, send_sems.at[k]).wait()

        pl.when(my_x == 0)(lambda: column(0))
        pl.when(my_x == 1)(lambda: column(1))

    return pl.pallas_call(
        body,
        out_shape=pltpu.VMEM((2 * m, n), x.dtype),
        in_specs=[pl.BlockSpec(memory_space=pl.ANY)],
        out_specs=pl.BlockSpec(memory_space=pltpu.VMEM),
        scratch_shapes=[
            pltpu.VMEM((2 * m, n), jnp.bfloat16),
            pltpu.SemaphoreType.DMA((len(groups) + 1,)),
            pltpu.SemaphoreType.DMA((2,)),
            pltpu.SemaphoreType.DMA((len(chunks),)),
            pltpu.SemaphoreType.DMA((n_fwd,)),
            pltpu.SemaphoreType.REGULAR,
        ],
        compiler_params=pltpu.CompilerParams(
            collective_id=0, disable_semaphore_checks=True
        ),
    )(x)
```

```python
import jax
import jax.numpy as jnp
from jax import lax
from jax.experimental import pallas as pl
from jax.experimental.pallas import tpu as pltpu

_MESH = pl.DeviceIdType.MESH

_TILE = 16
_FWD_ROWS = 464
_LOAD_ROWS = (16, 16, 32, 96)
_SEND_AHEAD = 160
_X_LAG = 96


def _schedule(m, n):
    f, t, h = _FWD_ROWS, _TILE, n // 2
    fwd = [(r, t, col, h) for r in range(0, f, t) for col in (0, h)] + [(f, t, 0, h)]
    both = [
        (f, t, h, h),
        (f + t, m - 2 * f - 3 * t, 0, n),
        (m - f - 2 * t, t, 0, n),
        (m - f - t, t, h, h),
    ]
    events, time = [], 0
    for i, (_, rows, _, cols) in enumerate(fwd + both):
        events.append((time - _SEND_AHEAD, 1, "send_y", i))
        time += rows * cols // n
        events.append((time, 0, "recv_y", i))
        if i < len(fwd):
            events.append((time + _X_LAG, 2, "recv_x", i))
    return fwd + both, len(fwd), [(kind, i) for _, _, kind, i in sorted(events)]


def pallas_dist_ag_xy_y_m1024_n512_kernel(x: jax.Array):
    m, n = x.shape
    chunks, n_fwd, events = _schedule(m, n)

    groups, start = {}, 0
    for rows in _LOAD_ROWS + (m - _FWD_ROWS - sum(_LOAD_ROWS),):
        groups[min(i for i, c in enumerate(chunks) if c[0] >= start)] = (start, rows)
        start += rows

    def body(x_ref, o_ref, buf, load_sems, send_sems, y_sems, x_sems, x_ready):
        my_x, my_y = lax.axis_index("x"), lax.axis_index("y")
        own, other = my_y * m, (1 - my_y) * m
        barrier = pltpu.get_barrier_semaphore()

        def column(cx):
            y_nbr, x_nbr = (cx, 1 - my_y), (1 - cx, my_y)

            def row(col, s, c):
                return s if col == 0 else m - s - c

            def at(base, r, c):
                return pl.ds(pl.multiple_of(base + r, _TILE), c)

            def load(r, c, k):
                return pltpu.make_async_copy(
                    x_ref.at[pl.ds(r, c)], o_ref.at[at(own, r, c)], load_sems.at[k]
                )

            def remote(idx, send_sem, recv_sem, nbr):
                return pltpu.make_async_remote_copy(
                    buf.at[idx], buf.at[idx], send_sem, recv_sem,
                    device_id=nbr, device_id_type=_MESH,
                )

            loads = {
                i: load(row(cx, s, c), c, k) for k, (i, (s, c)) in enumerate(groups.items())
            }
            *early_loads, late_load = loads.values()
            unsent_load = load(row(1 - cx, 0, _FWD_ROWS), _FWD_ROWS, len(groups))
            for copy in early_loads:
                copy.start()

            pl.semaphore_signal(barrier, 1, device_id=y_nbr, device_id_type=_MESH)
            if cx == 0:
                pl.semaphore_signal(barrier, 1, device_id=x_nbr, device_id_type=_MESH)

            last_send = {}
            for kind, i in events:
                s, c, col, cols = chunks[i]
                cols = pl.ds(col, cols)
                y_send = send_sems.at[2 if i == len(chunks) - 1 else 0]
                x_send = send_sems.at[3 if i == n_fwd - 1 else 1]
                if kind == "send_y":
                    idx = (at(own, row(cx, s, c), c), cols)
                    if i in loads:
                        loads[i].wait()
                    if i == 0:
                        late_load.start()
                        unsent_load.start()
                    buf[idx] = o_ref[idx].astype(jnp.bfloat16)
                    if i == 0:
                        pl.semaphore_wait(barrier, 1 + cx)
                    last_send["y"] = remote(idx, y_send, y_sems.at[i], y_nbr)
                    last_send["y"].start()
                    if i == 0 and cx == 1:
                        pl.semaphore_signal(
                            x_ready, 1, device_id=x_nbr, device_id_type=_MESH
                        )
                    continue
                if kind == "recv_y":
                    idx = (at(other, row(cx, s, c), c), cols)
                    if i == 0 and cx == 0:
                        pl.semaphore_wait(x_ready, 1)
                    remote(idx, y_send, y_sems.at[i], y_nbr).wait_recv()
                    if i < n_fwd:
                        last_send["x"] = remote(idx, x_send, x_sems.at[i], x_nbr)
                        last_send["x"].start()
                else:
                    idx = (at(other, row(1 - cx, s, c), c), cols)
                    remote(idx, x_send, x_sems.at[i], x_nbr).wait_recv()
                o_ref[idx] = buf[idx].astype(o_ref.dtype)

            unsent_load.wait()
            whole = ((own, m - _FWD_ROWS - _TILE), (other, _FWD_ROWS))
            for k, (base, c) in enumerate(whole):
                sent = buf.at[at(base, row(cx, 0, c), c)]
                pltpu.make_async_copy(sent, sent, send_sems.at[k]).wait()
            last_send["y"].wait_send()
            last_send["x"].wait_send()

        pl.when(my_x == 0)(lambda: column(0))
        pl.when(my_x == 1)(lambda: column(1))

    return pl.pallas_call(
        body,
        out_shape=pltpu.VMEM((2 * m, n), x.dtype),
        in_specs=[pl.BlockSpec(memory_space=pl.ANY)],
        out_specs=pl.BlockSpec(memory_space=pltpu.VMEM),
        scratch_shapes=[
            pltpu.VMEM((2 * m, n), jnp.bfloat16),
            pltpu.SemaphoreType.DMA((len(groups) + 1,)),
            pltpu.SemaphoreType.DMA((4,)),
            pltpu.SemaphoreType.DMA((len(chunks),)),
            pltpu.SemaphoreType.DMA((n_fwd,)),
            pltpu.SemaphoreType.REGULAR,
        ],
        compiler_params=pltpu.CompilerParams(
            collective_id=0, disable_semaphore_checks=True
        ),
    )(x)
```
